```python
import numpy as np

kernel_name = "dist_mean_ax0_shard0_i_m1024_n512"

def setup_inputs():
    return {"x": np.random.randn(4096, 512).astype(np.float32)}

def reference(x: np.ndarray) -> np.ndarray:
    return np.mean(x, axis=0, keepdims=True)
```

```python
import jax
import jax.numpy as jnp
from jax import lax
from jax.experimental import pallas as pl
from jax.experimental.pallas import tpu as pltpu

N_DEV = 4
N_CHUNKS = 8


def pallas_dist_mean_ax0_shard0_i_m1024_n512_kernel(
    x: jax.Array,
):
    m, n = x.shape
    rows = m // N_CHUNKS
    inv_total = 1.0 / float(m * N_DEV)

    def body(x_hbm, out_ref, xbuf, comm, load_sems, send_sems, recv_sems):
        me = lax.axis_index("i")

        loads = []
        for c in range(N_CHUNKS):
            cp = pltpu.make_async_copy(
                x_hbm.at[pl.ds(c * rows, rows), :],
                xbuf.at[pl.ds(c * rows, rows), :],
                load_sems.at[c],
            )
            cp.start()
            loads.append(cp)

        barrier = pltpu.get_barrier_semaphore()
        for d in range(1, N_DEV):
            pl.semaphore_signal(
                barrier,
                inc=1,
                device_id=((me + d) % N_DEV,),
                device_id_type=pl.DeviceIdType.MESH,
            )

        acc = jnp.zeros((8, n), jnp.float32)
        for c in range(N_CHUNKS):
            loads[c].wait()
            blk = xbuf[pl.ds(c * rows, rows), :]
            acc = acc + jnp.sum(blk.reshape(rows // 8, 8, n), axis=0)
        part = jnp.sum(acc, axis=0, keepdims=True)
        comm[0] = part

        pl.semaphore_wait(barrier, N_DEV - 1)

        rdmas = []
        for d in range(1, N_DEV):
            rdma = pltpu.make_async_remote_copy(
                src_ref=comm.at[0],
                dst_ref=comm.at[d],
                send_sem=send_sems.at[d - 1],
                recv_sem=recv_sems.at[d - 1],
                device_id=((me + d) % N_DEV,),
                device_id_type=pl.DeviceIdType.MESH,
            )
            rdma.start()
            rdmas.append(rdma)

        total = part
        for d in range(1, N_DEV):
            rdmas[d - 1].wait_recv()
            total = total + comm[d]
        out_ref[...] = total * inv_total
        for d in range(1, N_DEV):
            rdmas[d - 1].wait_send()

    return pl.pallas_call(
        body,
        out_shape=jax.ShapeDtypeStruct((1, n), jnp.float32),
        in_specs=[pl.BlockSpec(memory_space=pl.ANY)],
        out_specs=pl.BlockSpec(memory_space=pltpu.VMEM),
        scratch_shapes=[
            pltpu.VMEM((m, n), jnp.float32),
            pltpu.VMEM((N_DEV, 1, n), jnp.float32),
            pltpu.SemaphoreType.DMA((N_CHUNKS,)),
            pltpu.SemaphoreType.DMA((N_DEV - 1,)),
            pltpu.SemaphoreType.DMA((N_DEV - 1,)),
        ],
        compiler_params=pltpu.CompilerParams(collective_id=0),
    )(x)
```

```python
import jax
import jax.numpy as jnp
from jax import lax
from jax.experimental import pallas as pl
from jax.experimental.pallas import tpu as pltpu

N_DEV = 4
LATE = 2
K_RAW = 40
TAIL = 96
N_E = 128


def _colsum8(v):
    rows, w = v.shape
    g = rows // 8
    k = 1
    while k < 8 and g % (2 * k) == 0 and (2 * k) * (w // 128) <= 8:
        k *= 2
    acc = jnp.sum(v.reshape(g // k, k * 8, w), axis=0)
    while k > 1:
        k //= 2
        acc = acc[: k * 8] + acc[k * 8:]
    return acc


def _compiler_params():
    try:
        return pltpu.CompilerParams(collective_id=0, disable_semaphore_checks=True)
    except TypeError:
        return pltpu.CompilerParams(collective_id=0)


def pallas_dist_mean_ax0_shard0_i_m1024_n512_kernel(
    x: jax.Array,
):
    m, n = x.shape
    n_m = n - N_E
    inv_total = 1.0 / float(m * N_DEV)
    r0 = 2 * K_RAW
    r1 = m - TAIL

    def body(x_hbm, out_ref, xbuf, mbuf, ebuf, rawbuf, msrc, esrc, mrcv, ercv,
             fsrc, frcv, load_sems, send_sems, recv_sems, raw_send, raw_recv):
        me = lax.axis_index("i")
        is_late = me == LATE

        ld_bulk = pltpu.make_async_copy(
            x_hbm.at[pl.ds(r0, r1 - r0), :], xbuf.at[pl.ds(r0, r1 - r0), :],
            load_sems.at[0])
        ld_head = pltpu.make_async_copy(
            x_hbm.at[pl.ds(0, r0), :], xbuf.at[pl.ds(0, r0), :],
            load_sems.at[1])
        ld_m = pltpu.make_async_copy(
            x_hbm.at[pl.ds(r1, TAIL), pl.ds(0, n_m)], mbuf, load_sems.at[2])
        ld_e = pltpu.make_async_copy(
            x_hbm.at[pl.ds(r1, TAIL), pl.ds(n_m, N_E)], ebuf, load_sems.at[3])

        def raw(j):
            return pltpu.make_async_remote_copy(
                src_ref=x_hbm.at[pl.ds(j * K_RAW, K_RAW), :],
                dst_ref=rawbuf,
                send_sem=raw_send.at[j],
                recv_sem=raw_recv,
                device_id=(LATE ^ (1 + 2 * j),),
                device_id_type=pl.DeviceIdType.MESH,
            )

        def msg(k):
            src, dst, d = (
                (msrc, mrcv, 2),
                (esrc, ercv, 2),
                (fsrc, frcv.at[0], 1),
                (fsrc, frcv.at[1], 3),
            )[k]
            return pltpu.make_async_remote_copy(
                src_ref=src,
                dst_ref=dst,
                send_sem=send_sems.at[k],
                recv_sem=recv_sems.at[k],
                device_id=(me ^ d,),
                device_id_type=pl.DeviceIdType.MESH,
            )

        ld_bulk.start()
        barrier = pltpu.get_barrier_semaphore()
        for d in (1, 3, 2):
            pl.semaphore_signal(
                barrier, inc=1, device_id=(me ^ d,),
                device_id_type=pl.DeviceIdType.MESH)

        @pl.when(jnp.logical_not(is_late))
        def _():
            ld_head.start()

        ld_m.start()
        ld_e.start()

        pl.semaphore_wait(barrier, N_DEV - 1)

        def reduce_and_send(role):
            if role == "late":
                raw(0).start()
                raw(1).start()
                ld_bulk.wait()
                acc = _colsum8(xbuf[pl.ds(r0, r1 - r0), :])
            else:
                ld_head.wait()
                ld_bulk.wait()
                acc = _colsum8(xbuf[pl.ds(0, r1), :])
            if role == "helper":
                raw(0).wait_recv()
                acc = acc + _colsum8(rawbuf[...])
            ld_m.wait()
            part_m = jnp.sum(acc[:, :n_m] + _colsum8(mbuf[...]),
                             axis=0, keepdims=True)
            msrc[...] = part_m
            msg(0).start()
            ld_e.wait()
            part_e = jnp.sum(acc[:, n_m:] + _colsum8(ebuf[...]),
                             axis=0, keepdims=True)
            esrc[...] = part_e
            msg(1).start()
            fsrc[...] = jnp.concatenate([part_m, part_e], axis=1)
            msg(2).start()
            msg(3).start()

        @pl.when(is_late)
        def _():
            reduce_and_send("late")

        @pl.when((me ^ LATE) % 2 == 1)
        def _():
            reduce_and_send("helper")

        @pl.when(me == LATE ^ 2)
        def _():
            reduce_and_send("plain")

        msg(2).wait_recv()
        msg(3).wait_recv()
        near = fsrc[...] + frcv[0] + frcv[1]
        for k in range(4):
            msg(k).wait_send()

        @pl.when(is_late)
        def _():
            raw(0).wait_send()
            raw(1).wait_send()

        msg(0).wait_recv()
        out_ref[:, pl.ds(0, n_m)] = (near[:, :n_m] + mrcv[...]) * inv_total
        msg(1).wait_recv()
        out_ref[:, pl.ds(n_m, N_E)] = (near[:, n_m:] + ercv[...]) * inv_total

    return pl.pallas_call(
        body,
        out_shape=jax.ShapeDtypeStruct((1, n), jnp.float32),
        in_specs=[pl.BlockSpec(memory_space=pl.ANY)],
        out_specs=pl.BlockSpec(memory_space=pltpu.VMEM),
        scratch_shapes=[
            pltpu.VMEM((r1, n), jnp.float32),
            pltpu.VMEM((TAIL, n_m), jnp.float32),
            pltpu.VMEM((TAIL, N_E), jnp.float32),
            pltpu.VMEM((K_RAW, n), jnp.float32),
            pltpu.VMEM((1, n_m), jnp.float32),
            pltpu.VMEM((1, N_E), jnp.float32),
            pltpu.VMEM((1, n_m), jnp.float32),
            pltpu.VMEM((1, N_E), jnp.float32),
            pltpu.VMEM((1, n), jnp.float32),
            pltpu.VMEM((2, 1, n), jnp.float32),
            pltpu.SemaphoreType.DMA((4,)),
            pltpu.SemaphoreType.DMA((4,)),
            pltpu.SemaphoreType.DMA((4,)),
            pltpu.SemaphoreType.DMA((2,)),
            pltpu.SemaphoreType.DMA,
        ],
        compiler_params=_compiler_params(),
    )(x)
```
